```python
import numpy as np

kernel_name = "dist_pipemlp_pp2tp2_xy_b4096_d256_h512"

def setup_inputs():
    x_padded = np.zeros((2, 4096, 256), dtype=np.float32)
    x_padded[0] = np.random.randn(4096, 256).astype(np.float32)
    Win = np.random.randn(4, 256, 1024).astype(np.float32)
    Wout = np.random.randn(4, 1024, 256).astype(np.float32)
    return {"x_padded": x_padded, "Win": Win, "Wout": Wout}

def reference(x_padded, Win, Wout):
    a = x_padded[0]
    for k in range(4):
        h = a @ Win[k]
        h = np.maximum(h, 0.0)
        a = h @ Wout[k]
    out = np.zeros_like(x_padded)
    out[1] = a
    return out
```

```python
import jax
import jax.numpy as jnp
from jax import lax
from jax.experimental import pallas as pl
from jax.experimental.pallas import tpu as pltpu

_MESH = pl.DeviceIdType.MESH
_BF16 = jnp.bfloat16
_F32 = jnp.float32
_TILE = 16

_CFG = dict(
    own=(32,) + (112,) * 6 + (80,) * 12,
    shared=(80,) * 9 + (48,),
    off=(11, 12, 14, 15, 17, 18, 20, 21, 23, 24, 26, 27, 28),
    merged=(1, 8, 10, 12, 15, 18, 21, 24),
    k_pre=7,
    j_mid=(13, 14),
    groups=((9, 19), (17, 27), (19, 29)),
    cuts=(32, 96),
    n_blk=4,
    n_slice=6,
)


def _schedule(cfg):
    sizes = cfg["own"] + cfg["shared"]
    n_own, n_seq = len(cfg["own"]), len(sizes)
    start = [sum(sizes[:j]) for j in range(n_seq + 1)]
    off, k_pre = cfg["off"], cfg["k_pre"]
    heads = [j for j in range(n_seq + 1) if j not in cfg["merged"]]
    units = dict(zip(heads, heads[1:]))
    assert all(j in heads for j in (0, n_own, k_pre))
    assert all((j in off) == (j - 1 in off) for j in cfg["merged"])
    assert max(k_pre, 1 + cfg["n_slice"]) <= min(off)

    sem, extra = {0: n_seq}, {}

    def step(name, a, b):
        return (name, sizes[a:b]), start[a], a, sem.get(a, -1)

    for kind, due in zip(("far_mid", "near_mid"), cfg["j_mid"]):
        extra.setdefault(due, []).append(step(kind, 0, units[0]))
    n_sem, lo = n_seq + 1, units[0]
    for hi, due in cfg["groups"]:
        assert lo < hi and hi in heads
        sem.update({j: n_sem for j in range(lo, hi)})
        kind = ("results", (start[hi] - start[lo],))
        extra.setdefault(due, []).append((kind, start[lo], lo, n_sem))
        n_sem, lo = n_sem + 1, hi
    assert lo == n_own and all(k_pre <= due and due in heads for due in extra)

    stream = []
    for a, b in units.items():
        if a >= k_pre:
            stream += extra.get(a, []) + [step("layer3" if a in off else "layers23", a, b)]
    early = [step("layer1_slice" if 1 <= j <= cfg["n_slice"] else "layer1", j, j + 1)
             for j in range(min(off))]
    late = [step("layers12" if j in off else "layer1", j, j + 1) for j in range(min(off), n_seq)]
    pre = [step("pre" if a else "pre_mid", a, b) for a, b in units.items() if a < k_pre]
    backlog = [step("backlog", a, b) for a, b in units.items() if 0 < a < k_pre]
    return (early, late), (pre, backlog + stream + extra.get(n_seq, [])), n_sem


def _repeat(kinds):
    best = (1, 1)
    for period in range(1, len(kinds) // 2 + 1):
        count = 1
        while kinds[count * period:(count + 1) * period] == kinds[:period]:
            count += 1
        if count > 1 and count * period > best[0] * best[1]:
            best = (period, count)
    return best


def _make_body(batch, d, hid, cfg):
    sizes = cfg["own"] + cfg["shared"]
    n_own, n_seq, n_blk = len(cfg["own"]), len(sizes), cfg["n_blk"]
    own_rows, seq_rows = sum(cfg["own"]), sum(sizes)
    assert own_rows + seq_rows == batch and all(s % _TILE == 0 for s in sizes)
    assert n_blk >= 3 and batch % (2 * n_blk * _TILE) == 0
    blk_rows, slice_rows = own_rows // n_blk, (seq_rows - own_rows) // cfg["n_slice"]
    assert own_rows % (n_blk * _TILE) == 0
    assert (seq_rows - own_rows) % (cfg["n_slice"] * _TILE) == 0
    cuts = (0,) + cfg["cuts"] + (d,)
    plan0, plan1, n_sem = _schedule(cfg)
    mid_rows = sum(plan1[0][0][0][1])
    n_steps = max(len(a) + len(b) for a, b in (plan0, plan1))

    def body(x_hbm, win_hbm, wout_hbm, out_ref,
             wi32, wo32, wi, wo, x32, acc, y_send, y_recv, x_send, x_recv, mid, far, table,
             ready, w_sem, x_sem, swap_sent, up_sent, rows_sent, swap_sem, up_sem, recv_sem):
        mx = lax.axis_index("x")
        my = lax.axis_index("y")
        y_peer = (mx, 1 - my)
        x_peer = (1 - mx, my)

        barrier = pltpu.get_barrier_semaphore()
        pl.semaphore_signal(barrier, inc=1, device_id=y_peer, device_id_type=_MESH)

        @pl.when(mx == 0)
        def _():
            pl.semaphore_signal(barrier, inc=1, device_id=x_peer, device_id_type=_MESH)

        def rows(first, n):
            return pl.ds(first if isinstance(first, int) else pl.multiple_of(first, _TILE), n)

        def alone(fn):
            pl.when(my < 2)(fn)

        class Step:
            def __init__(self, parts, first, j, sem):
                self.j, self.sem, self.n = j, sem, sum(parts)
                self.first, self.seq = first, rows(first, sum(parts))
                self.parts = [(j + k, rows(first + sum(parts[:k]), n)) for k, n in enumerate(parts)]

            def batch(self, col):
                base = jnp.where(self.first < own_rows, col * own_rows, own_rows)
                return rows(base + self.first, self.n)

        def fill_table(steps):
            for i, (_, *values) in enumerate(steps):
                for k, value in enumerate(values):
                    table[3 * i + k] = value

        def run(kinds, base, fns):
            i = 0
            while i < len(kinds):
                period, count = _repeat(kinds[i:])
                if count == 1:
                    alone(lambda: run_step(kinds[i], base + i, fns))
                elif period == 1:
                    pl.loop(0, count)(lambda n: run_step(kinds[i], base + i + n, fns))
                else:
                    pl.loop(0, count)(
                        lambda n: run(kinds[i:i + period], base + i + n * period, fns))
                i += period * count

        def run_step(kind, i, fns):
            fns[kind[0]](Step(kind[1], *(table[3 * i + k] for k in range(3))))

        def own_piece(ref_in, ref_out, p):
            if p < 3:
                return ref_in, pl.ds(cuts[p], cuts[p + 1] - cuts[p])
            return ref_out, pl.ds(0, hid)

        def w_piece(slot, h, p):
            if p < 3:
                return wi.at[slot, pl.ds(cuts[p], cuts[p + 1] - cuts[p]), pl.ds(h * hid, hid)]
            return wo.at[slot, pl.ds(h * hid, hid)]

        def w_load(l, p):
            src, sl = own_piece(win_hbm, wout_hbm, p)
            dst, _ = own_piece(wi32, wo32, p)
            return pltpu.make_async_copy(src.at[l, sl], dst.at[l, sl], w_sem.at[4 * l + p])

        def w_cast(l, p):
            w_load(l, p).wait()
            src, sl = own_piece(wi32, wo32, p)
            w_piece(l, 0, p)[...] = src[l, sl, :].astype(_BF16)

        def remote(src, dst, send_sem, recv_sem, peer):
            return pltpu.make_async_remote_copy(
                src, dst, send_sem, recv_sem, device_id=peer, device_id_type=_MESH)

        def w_half(slot, h, i):
            sl = pl.ds(h * hid, hid)
            return wo.at[slot, sl] if i else wi.at[slot, :, sl]

        def w_swap(l, p):
            k = 2 * l + p // 3
            return remote(w_piece(l, 0, p), w_piece(l, 1, p), swap_sent.at[k], swap_sem.at[k], y_peer)

        def w_swapped(l, i):
            k = 2 * l + i
            return remote(w_half(l, 0, i), w_half(l, 1, i), swap_sent.at[k], swap_sem.at[k], y_peer)

        def w_up(h, p):
            k = p // 3
            return remote(w_piece(0, h, p), w_piece(2, h, p), up_sent.at[k], up_sem.at[k], x_peer)

        def w_upped(i):
            w = (wi, wo)[i]
            return remote(w.at[0], w.at[2], up_sent.at[i], up_sem.at[i], x_peer)

        def hidden(a, w):
            return jnp.maximum(jnp.dot(a, w, preferred_element_type=_F32), 0.0).astype(_BF16)

        def project(t, w):
            return jnp.dot(t, w, preferred_element_type=_F32)

        def half_layer(a, slot, h):
            return project(hidden(a, w_half(slot, h, 0)[...]), w_half(slot, h, 1)[...])

        def layer(a, slot):
            return project(hidden(a, wi[slot]), wo[slot])

        def x_copy(j, r):
            return remote(x_send.at[r], x_recv.at[r], rows_sent.at[0], recv_sem.at[j], x_peer)

        @pl.when(mx == 0)
        def _():
            def x_load(r, sem):
                return pltpu.make_async_copy(x_hbm.at[0, r], x32.at[r], x_sem.at[sem])

            def block_load(i):
                col = jnp.where(i >= n_blk, my, 1 - my)
                r = rows(col * own_rows + i % n_blk * blk_rows, blk_rows)
                return r, x_load(r, i % 3)

            shared_load = x_load(rows(2 * own_rows, batch - 2 * own_rows), 3)

            def partial(r):
                return half_layer(x32[r, :].astype(_BF16), 0, 0)

            def partial_copy(c, shared=0):
                return remote(y_send.at[c.batch(1 - my)], y_recv.at[c.seq],
                              rows_sent.at[1 + shared], recv_sem.at[c.j], y_peer)

            def partial_sends(lo, hi):
                steps = [Step(sizes[j:j + 1], sum(sizes[:j]), j, None) for j in range(lo, hi)]
                for c in steps:
                    partial_copy(c, c.j >= n_own).start()

            w_load(1, 0).start()
            w_load(1, 1).start()
            w_cast(1, 0)
            w_load(1, 2).start()
            for p in range(4):
                w_load(0, p).start()
            block_load(0)[1].start()
            pl.semaphore_wait(barrier, 1)
            w_swap(1, 0).start()
            w_cast(1, 1)
            w_swap(1, 1).start()
            w_cast(1, 2)
            w_swap(1, 2).start()
            fill_table(plan0[0] + plan0[1])
            for p in range(4):
                w_cast(0, p)
            block_load(1)[1].start()
            w_load(1, 3).start()

            def block(i, dst):
                r, load = block_load(i)
                load.wait()
                dst[r, :] = partial(r).astype(dst.dtype)
                n = batch // (2 * n_blk)
                out_ref[0, rows(i * n, n), :] = jnp.zeros((n, d), _F32)

            @pl.loop(0, n_blk)
            def _(i):
                block_load(i + 2)[1].start()
                block(i, y_send)

                @pl.when(i == 1)
                def _():
                    w_cast(1, 3)
                    w_swap(1, 3).start()

            shared_load.start()

            @alone
            def _():
                block_load(n_blk + 2)[1].start()
                partial_sends(0, n_own)
                block(n_blk, acc)

            @pl.loop(n_blk + 1, 2 * n_blk)
            def _(i):
                pl.when(i + 2 < 2 * n_blk)(lambda: block_load(i + 2)[1].start())
                block(i, acc)

            shared_load.wait()

            pl.semaphore_wait(ready, 1)
            w_swapped(1, 0).wait_recv()
            w_swapped(1, 1).wait_recv()

            def stage0(c, n_layers):
                near = acc[c.batch(my), :]
                partial_copy(c).wait_recv()
                a = (near + y_recv[c.seq, :].astype(_F32)).astype(_BF16)
                for slot in range(1, 1 + n_layers):
                    a = layer(a, slot).astype(_BF16)
                x_send[c.seq, :] = a
                x_copy(c.j, c.seq).start()

            def stage0_and_slice(c):
                stage0(c, 1)

                @alone
                def _():
                    r = rows(2 * own_rows + (c.j - 1) * slice_rows, slice_rows)
                    part = partial(r)
                    acc[r, :] = part
                    y_send[r, :] = part.astype(_BF16)

                pl.when(c.j == cfg["n_slice"])(lambda: partial_sends(n_own, n_seq))

            fns = dict(layer1=lambda c: stage0(c, 1), layers12=lambda c: stage0(c, 2),
                       layer1_slice=stage0_and_slice)
            run([step[0] for step in plan0[0]], 0, fns)
            w_upped(0).wait_recv()
            w_upped(1).wait_recv()
            run([step[0] for step in plan0[1]], len(plan0[0]), fns)

        @pl.when(mx == 1)
        def _():
            pieces = [(l, p) for l in range(2) for p in range(4)]
            w_load(0, 0).start()
            w_load(0, 1).start()
            w_cast(0, 0)
            for l, p in pieces[2:4]:
                w_load(l, p).start()
            pl.semaphore_wait(barrier, 2)
            for l, p in pieces:
                if (l, p) != (0, 0):
                    w_cast(l, p)
                w_swap(l, p).start()
                if l == 0:
                    w_up(0, p).start()
                    w_load(1, p).start()
            pl.semaphore_signal(ready, inc=1, device_id=x_peer, device_id_type=_MESH)
            w_swapped(0, 0).wait_recv()
            for p in range(3):
                w_up(1, p).start()
            w_swapped(0, 1).wait_recv()
            w_up(1, 3).start()

            def y_copy(c, src):
                return remote(src.at[c.seq], y_recv.at[c.seq],
                              rows_sent.at[2 if src is mid else 1], recv_sem.at[c.sem], y_peer)

            def arrived(c):
                for part in c.parts:
                    x_copy(*part).wait_recv()
                return x_recv[c.seq, :]

            def pre_mid(c):
                a = layer(arrived(c), 0).astype(_BF16)
                mid[c.seq, :] = a
                acc[c.seq, :] = half_layer(a, 1, 0)
                y_copy(c, mid).start()

            def pre(c):
                a = layer(arrived(c), 0).astype(_BF16)
                t = hidden(a, wi[1])
                far[c.seq, :] = t[:, hid:]
                acc[c.seq, :] = project(t[:, :hid], w_half(1, 0, 1)[...])

            def backlog(c):
                finish(c, acc[c.seq, :] + project(far[c.seq, :], w_half(1, 1, 1)[...]))

            def finish(c, res):
                out_ref[0, c.batch(my), :] = res
                y_send[c.seq, :] = res.astype(_BF16)
                pl.when(c.first < own_rows)(lambda: y_copy(c, y_send).start())

            def near_mid(c):
                out_ref[0, c.batch(my), :] = acc[c.seq, :] + half_layer(mid[c.seq, :], 1, 1)

            def far_mid(c):
                y_copy(c, y_recv).wait_recv()
                out_ref[0, c.batch(1 - my), :] = layer(y_recv[c.seq, :], 1)

            def results(c):
                y_copy(c, y_recv).wait_recv()
                out_ref[0, c.batch(1 - my), :] = y_recv[c.seq, :].astype(_F32)

            fns = dict(
                pre_mid=pre_mid, pre=pre, backlog=backlog,
                near_mid=near_mid, far_mid=far_mid, results=results,
                layer3=lambda c: finish(c, layer(arrived(c), 1)),
                layers23=lambda c: finish(c, layer(layer(arrived(c), 0).astype(_BF16), 1)))
            fill_table(plan1[0] + plan1[1])
            run([plan1[0][0][0]], 0, fns)
            w_swapped(1, 0).wait_recv()
            run([step[0] for step in plan1[0][1:]], 1, fns)
            w_swapped(1, 1).wait_recv()
            run([step[0] for step in plan1[1]], len(plan1[0]), fns)

        def sent(ref, first, n, k):
            ref = ref.at[rows(first, n)]
            remote(ref, ref, rows_sent.at[k], recv_sem.at[0], y_peer).wait_send()

        @pl.when(mx == 0)
        def _():
            for i in range(2):
                w_swapped(1, i).wait_send()
            sent(y_send, (1 - my) * own_rows, own_rows, 1)
            sent(y_send, 2 * own_rows, batch - 2 * own_rows, 2)
            sent(x_send, 0, seq_rows, 0)

        @pl.when(mx == 1)
        def _():
            for i in range(2):
                w_upped(i).wait_send()
                w_swapped(0, i).wait_send()
                w_swapped(1, i).wait_send()
            sent(mid, 0, mid_rows, 2)
            sent(y_send, mid_rows, own_rows - mid_rows, 1)

    dma = pltpu.SemaphoreType.DMA
    scratch = [
        pltpu.VMEM((2, d, hid), _F32),
        pltpu.VMEM((2, hid, d), _F32),
        pltpu.VMEM((3, d, 2 * hid), _BF16),
        pltpu.VMEM((3, 2 * hid, d), _BF16),
        pltpu.VMEM((batch, d), _F32),
        pltpu.VMEM((batch, d), _F32),
        pltpu.VMEM((batch, d), _BF16),
        pltpu.VMEM((seq_rows, d), _BF16),
        pltpu.VMEM((seq_rows, d), _BF16),
        pltpu.VMEM((seq_rows, d), _BF16),
        pltpu.VMEM((mid_rows, d), _BF16),
        pltpu.VMEM((sum(sizes[:cfg["k_pre"]]), hid), _BF16),
        pltpu.SMEM((3 * n_steps,), jnp.int32),
        pltpu.SemaphoreType.REGULAR,
        dma((8,)), dma((4,)),
        dma((4,)), dma((2,)), dma((3,)),
        dma((4,)), dma((2,)), dma((n_sem,)),
    ]
    return body, scratch


def _run(x_padded, Win, Wout, cfg):
    _, batch, d = x_padded.shape
    hid = Win.shape[2]
    body, scratch = _make_body(batch, d, hid, cfg)
    return pl.pallas_call(
        body,
        out_shape=jax.ShapeDtypeStruct(x_padded.shape, x_padded.dtype),
        in_specs=[pl.BlockSpec(memory_space=pltpu.HBM)] * 3,
        out_specs=pl.BlockSpec(memory_space=pltpu.VMEM),
        scratch_shapes=scratch,
        compiler_params=pltpu.CompilerParams(
            collective_id=0, vmem_limit_bytes=64 * 1024 * 1024,
            disable_semaphore_checks=True),
    )(x_padded, Win, Wout)


def pallas_dist_pipemlp_pp2tp2_xy_b4096_d256_h512_kernel(
    x_padded: jax.Array,
    Win: jax.Array,
    Wout: jax.Array,
):
    return _run(x_padded, Win, Wout, _CFG)
```
